```python
import numpy as np

kernel_name = "dist_rmsnorm_colshard_i_m768_n512"

def setup_inputs():
    x = np.random.randn(768, 2048).astype(np.float32)
    gamma = np.random.randn(2048).astype(np.float32)
    return {"x": x, "gamma": gamma}

def reference(x: np.ndarray, gamma: np.ndarray) -> np.ndarray:
    eps = 1e-5
    rms = np.sqrt(np.mean(x * x, axis=1, keepdims=True) + eps)
    return gamma * x / rms
```

```python
import jax
import jax.numpy as jnp
from jax import lax
from jax.experimental import pallas as pl
from jax.experimental.pallas import tpu as pltpu

N_DEV = 4
EPS = 1e-5

def pallas_dist_rmsnorm_colshard_i_m768_n512_kernel(x, gamma, chunks=(128,)*6, oshape="sds", scopes=False):
    m, n = x.shape
    nc = len(chunks)
    assert sum(chunks) == m
    offs = [sum(chunks[:i]) for i in range(nc)]
    n_global = n * N_DEV

    import contextlib
    def scope(name):
        return jax.named_scope(name) if scopes else contextlib.nullcontext()

    def body(x_hbm, g_hbm, o_ref, xbuf, gbuf, part, in_sems, g_sem, send_sems, recv_sems):
        in_copies = []
        for c in range(nc):
            cp = pltpu.make_async_copy(x_hbm.at[pl.ds(offs[c], chunks[c])], xbuf.at[pl.ds(offs[c], chunks[c])], in_sems.at[c])
            cp.start()
            in_copies.append(cp)
        gcp = pltpu.make_async_copy(g_hbm, gbuf, g_sem)
        gcp.start()
        my = lax.axis_index("i")
        barrier = pltpu.get_barrier_semaphore()
        for d in range(1, N_DEV):
            pl.semaphore_signal(barrier, inc=1, device_id=((my + d) % N_DEV,),
                                device_id_type=pl.DeviceIdType.MESH)

        lane = lax.broadcasted_iota(jnp.int32, (8, 128), 1)
        rdmas = []
        for c in range(nc):
            with scope(f"win{c}"):
                in_copies[c].wait()
            with scope(f"p1_{c}"):
                packed = jnp.zeros((8, 128), jnp.float32)
                for j in range(chunks[c] // 8):
                    xv = xbuf[pl.ds(offs[c] + j * 8, 8), :]
                    s = jnp.sum(xv * xv, axis=1, keepdims=True)
                    packed = jnp.where(lane == j, s, packed)
                part[0, c] = packed
            if c == 0:
                with scope("bar"):
                    pl.semaphore_wait(barrier, N_DEV - 1)
            for d in (2, 1, 3):
                r = pltpu.make_async_remote_copy(
                    src_ref=part.at[0, c], dst_ref=part.at[d, c],
                    send_sem=send_sems.at[d - 1, c], recv_sem=recv_sems.at[d - 1, c],
                    device_id=((my + d) % N_DEV,), device_id_type=pl.DeviceIdType.MESH)
                r.start()
                rdmas.append(r)

        gcp.wait()
        g = gbuf[...]
        for c in range(nc):
            with scope(f"wrecv{c}"):
                for d in range(1, N_DEV):
                    rdmas[c * (N_DEV - 1) + d - 1].wait_recv()
            with scope(f"p2_{c}"):
                tot = part[0, c] + part[1, c] + part[2, c] + part[3, c]
                inv = lax.rsqrt(tot * (1.0 / n_global) + EPS)
                for j in range(chunks[c] // 8):
                    sc = jnp.sum(jnp.where(lane == j, inv, 0.0), axis=1, keepdims=True)
                    xv = xbuf[pl.ds(offs[c] + j * 8, 8), :]
                    o_ref[pl.ds(offs[c] + j * 8, 8), :] = xv * sc * g
        with scope("wsend"):
            for r in rdmas:
                r.wait_send()

    out_shape = jax.ShapeDtypeStruct((m, n), x.dtype) if oshape == "sds" else pltpu.VMEM((m, n), x.dtype)
    return pl.pallas_call(
        body,
        out_shape=out_shape,
        in_specs=[pl.BlockSpec(memory_space=pl.ANY), pl.BlockSpec(memory_space=pl.ANY)],
        out_specs=pl.BlockSpec(memory_space=pltpu.VMEM),
        scratch_shapes=[
            pltpu.VMEM((m, n), jnp.float32),
            pltpu.VMEM((1, n), jnp.float32),
            pltpu.VMEM((N_DEV, nc, 8, 128), jnp.float32),
            pltpu.SemaphoreType.DMA((nc,)),
            pltpu.SemaphoreType.DMA,
            pltpu.SemaphoreType.DMA((N_DEV - 1, nc)),
            pltpu.SemaphoreType.DMA((N_DEV - 1, nc)),
        ],
        compiler_params=pltpu.CompilerParams(collective_id=0, disable_semaphore_checks=True),
    )(x, gamma.reshape(1, n))
```

```python
import jax
import jax.numpy as jnp
from jax import lax
from jax.experimental import pallas as pl
from jax.experimental.pallas import tpu as pltpu

N_DEV = 4
EPS = 1e-5
LANES = 128
SUBLANES = 8
MAX_CHUNK = 128
LEAD = 2


def _row_chunks(m):
    chunks = [MAX_CHUNK] * (m // MAX_CHUNK)
    if m % MAX_CHUNK:
        chunks.append(m % MAX_CHUNK)
    last = chunks[-1]
    if last % (2 * SUBLANES) == 0:
        chunks[-1:] = [last // 2, last // 2]
    return tuple(chunks)


def _compiler_params():
    try:
        return pltpu.CompilerParams(collective_id=0, disable_semaphore_checks=True)
    except TypeError:
        return pltpu.CompilerParams(collective_id=0)


def pallas_dist_rmsnorm_colshard_i_m768_n512_kernel(
    x: jax.Array,
    gamma: jax.Array,
):
    m, n = x.shape
    assert m % SUBLANES == 0 and n % LANES == 0
    chunks = _row_chunks(m)
    nc = len(chunks)
    offs = [sum(chunks[:c]) for c in range(nc)]
    groups = [r // SUBLANES for r in chunks]
    inv_n = 1.0 / (n * N_DEV)
    stride = LANES // SUBLANES

    def body(x_hbm, g_hbm, o_ref, xbuf, gbuf, part, diag, in_sems, g_sem,
             send_sem, recv_sems):
        in_copies = []
        for c in range(nc):
            rows = pl.ds(offs[c], chunks[c])
            cp = pltpu.make_async_copy(x_hbm.at[rows], xbuf.at[rows], in_sems.at[c])
            cp.start()
            in_copies.append(cp)
        g_copy = pltpu.make_async_copy(g_hbm, gbuf, g_sem)
        g_copy.start()

        my = lax.axis_index("i")
        peers = (2, 1, 3)
        barrier = pltpu.get_barrier_semaphore()
        for d in peers:
            pl.semaphore_signal(barrier, inc=1, device_id=((my + d) % N_DEV,),
                                device_id_type=pl.DeviceIdType.MESH)

        lane = lax.broadcasted_iota(jnp.int32, (SUBLANES, LANES), 1)
        sub = lax.broadcasted_iota(jnp.int32, (SUBLANES, LANES), 0)
        key = lane - stride * sub

        own = []
        rdmas = {}
        for c in range(nc):
            in_copies[c].wait()
            packed = jnp.zeros((SUBLANES, LANES), jnp.float32)
            for j in range(groups[c]):
                xv = xbuf[pl.ds(offs[c] + j * SUBLANES, SUBLANES), :]
                ss = jnp.sum(xv * xv, axis=1, keepdims=True)
                packed = jnp.where(key == j, ss, packed)
            row = jnp.sum(packed, axis=0, keepdims=True)
            own.append(row)
            part[0, c] = row
            if c == 0:
                pl.semaphore_wait(barrier, N_DEV - 1)
            for d in peers:
                dst = diag.at[c] if d == 2 else part.at[1 if d == 1 else 2, c]
                rdma = pltpu.make_async_remote_copy(
                    src_ref=part.at[0, c], dst_ref=dst,
                    send_sem=send_sem, recv_sem=recv_sems.at[d - 1, c],
                    device_id=((my + d) % N_DEV,),
                    device_id_type=pl.DeviceIdType.MESH)
                rdma.start()
                rdmas[c, d] = rdma

        g_copy.wait()
        g = gbuf[...]

        near = {}

        def add_neighbours(c):
            rdmas[c, 1].wait_recv()
            rdmas[c, 3].wait_recv()
            t = own[c] + part[1, c] + part[2, c]
            tb = jnp.broadcast_to(t, (SUBLANES, LANES))
            near[c] = [jnp.sum(jnp.where(key == j, tb, 0.0), axis=1, keepdims=True)
                       for j in range(groups[c])]

        def finish(c):
            rdmas[c, 2].wait_recv()
            for j in range(groups[c]):
                far = jnp.full((SUBLANES, LANES), diag[c, 0, j], jnp.float32)
                for s in range(1, SUBLANES):
                    far = jnp.where(sub == s, diag[c, 0, stride * s + j], far)
                inv_rms = lax.rsqrt((far + near[c][j]) * inv_n + EPS)
                rows = pl.ds(offs[c] + j * SUBLANES, SUBLANES)
                for k in range(n // LANES):
                    cols = pl.ds(k * LANES, LANES)
                    o_ref[rows, cols] = (
                        xbuf[rows, cols] * inv_rms * g[:, k * LANES:(k + 1) * LANES])

        n_added = 0
        for c in range(nc):
            while n_added < min(nc, c + 1 + LEAD):
                add_neighbours(n_added)
                n_added += 1
            finish(c)

        pltpu.make_async_copy(part, part, send_sem).wait()

    return pl.pallas_call(
        body,
        out_shape=jax.ShapeDtypeStruct((m, n), x.dtype),
        in_specs=[pl.BlockSpec(memory_space=pl.ANY),
                  pl.BlockSpec(memory_space=pl.ANY)],
        out_specs=pl.BlockSpec(memory_space=pltpu.VMEM),
        scratch_shapes=[
            pltpu.VMEM((m, n), jnp.float32),
            pltpu.VMEM((1, n), jnp.float32),
            pltpu.VMEM((N_DEV - 1, nc, 1, LANES), jnp.float32),
            pltpu.SMEM((nc, 1, LANES), jnp.float32),
            pltpu.SemaphoreType.DMA((nc,)),
            pltpu.SemaphoreType.DMA,
            pltpu.SemaphoreType.DMA,
            pltpu.SemaphoreType.DMA((N_DEV - 1, nc)),
        ],
        compiler_params=_compiler_params(),
    )(x, gamma.reshape(1, n))
```

```python
import jax
import jax.numpy as jnp
from jax import lax
from jax.experimental import pallas as pl
from jax.experimental.pallas import tpu as pltpu

N_DEV = 4
EPS = 1e-5
LANES = 128
SUBLANES = 8
MAX_CHUNK = 128
LEAD = 2


def _row_chunks(m):
    chunks = [MAX_CHUNK] * (m // MAX_CHUNK)
    if m % MAX_CHUNK:
        chunks.append(m % MAX_CHUNK)
    last = chunks[-1]
    if last % (2 * SUBLANES) == 0:
        chunks[-1:] = [last // 2, last // 2]
    return tuple(chunks)


def _compiler_params():
    try:
        return pltpu.CompilerParams(collective_id=0, disable_semaphore_checks=True)
    except TypeError:
        return pltpu.CompilerParams(collective_id=0)


def pallas_dist_rmsnorm_colshard_i_m768_n512_kernel(
    x: jax.Array,
    gamma: jax.Array,
):
    m, n = x.shape
    assert m % SUBLANES == 0 and n % LANES == 0
    chunks = _row_chunks(m)
    nc = len(chunks)
    offs = [sum(chunks[:c]) for c in range(nc)]
    groups = [r // SUBLANES for r in chunks]
    inv_n = 1.0 / (n * N_DEV)
    stride = LANES // SUBLANES

    def body(x_hbm, g_hbm, o_ref, xbuf, gbuf, part, diag, in_sems, g_sem,
             send_sems, recv_sems):
        in_copies = []
        for c in range(nc):
            rows = pl.ds(offs[c], chunks[c])
            cp = pltpu.make_async_copy(x_hbm.at[rows], xbuf.at[rows], in_sems.at[c])
            cp.start()
            in_copies.append(cp)
        g_copy = pltpu.make_async_copy(g_hbm, gbuf, g_sem)
        g_copy.start()

        my = lax.axis_index("i")
        peers = (2, 1, 3)
        barrier = pltpu.get_barrier_semaphore()
        for d in peers:
            pl.semaphore_signal(barrier, inc=1, device_id=((my + d) % N_DEV,),
                                device_id_type=pl.DeviceIdType.MESH)

        lane = lax.broadcasted_iota(jnp.int32, (SUBLANES, LANES), 1)
        sub = lax.broadcasted_iota(jnp.int32, (SUBLANES, LANES), 0)
        key = lane - stride * sub

        own = []
        rdmas = {}
        for c in range(nc):
            in_copies[c].wait()
            packed = jnp.zeros((SUBLANES, LANES), jnp.float32)
            for j in range(groups[c]):
                xv = xbuf[pl.ds(offs[c] + j * SUBLANES, SUBLANES), :]
                ss = jnp.sum(xv * xv, axis=1, keepdims=True)
                packed = jnp.where(key == j, ss, packed)
            row = jnp.sum(packed, axis=0, keepdims=True)
            own.append(row)
            part[0, c] = row
            if c == 0:
                pl.semaphore_wait(barrier, N_DEV - 1)
            for d in peers:
                dst = diag.at[c] if d == 2 else part.at[1 if d == 1 else 2, c]
                rdma = pltpu.make_async_remote_copy(
                    src_ref=part.at[0, c], dst_ref=dst,
                    send_sem=send_sems.at[d - 1, c], recv_sem=recv_sems.at[d - 1, c],
                    device_id=((my + d) % N_DEV,),
                    device_id_type=pl.DeviceIdType.MESH)
                rdma.start()
                rdmas[c, d] = rdma

        g_copy.wait()
        g = gbuf[...]

        near = {}

        def add_neighbours(c):
            rdmas[c, 1].wait_recv()
            rdmas[c, 3].wait_recv()
            t = own[c] + part[1, c] + part[2, c]
            tb = jnp.broadcast_to(t, (SUBLANES, LANES))
            near[c] = [jnp.sum(jnp.where(key == j, tb, 0.0), axis=1, keepdims=True)
                       for j in range(groups[c])]

        def finish(c):
            rdmas[c, 2].wait_recv()
            for j in range(groups[c]):
                far = jnp.full((SUBLANES, LANES), diag[c, 0, j], jnp.float32)
                for s in range(1, SUBLANES):
                    far = jnp.where(sub == s, diag[c, 0, stride * s + j], far)
                inv_rms = lax.rsqrt((far + near[c][j]) * inv_n + EPS)
                rows = pl.ds(offs[c] + j * SUBLANES, SUBLANES)
                for k in range(n // LANES):
                    cols = pl.ds(k * LANES, LANES)
                    o_ref[rows, cols] = (
                        xbuf[rows, cols] * inv_rms * g[:, k * LANES:(k + 1) * LANES])

        n_added = 0
        for c in range(nc):
            while n_added < min(nc, c + 1 + LEAD):
                add_neighbours(n_added)
                for d in peers:
                    rdmas[n_added, d].wait_send()
                n_added += 1
            finish(c)

    return pl.pallas_call(
        body,
        out_shape=jax.ShapeDtypeStruct((m, n), x.dtype),
        in_specs=[pl.BlockSpec(memory_space=pl.ANY),
                  pl.BlockSpec(memory_space=pl.ANY)],
        out_specs=pl.BlockSpec(memory_space=pltpu.VMEM),
        scratch_shapes=[
            pltpu.VMEM((m, n), jnp.float32),
            pltpu.VMEM((1, n), jnp.float32),
            pltpu.VMEM((N_DEV - 1, nc, 1, LANES), jnp.float32),
            pltpu.SMEM((nc, 1, LANES), jnp.float32),
            pltpu.SemaphoreType.DMA((nc,)),
            pltpu.SemaphoreType.DMA,
            pltpu.SemaphoreType.DMA((N_DEV - 1, nc)),
            pltpu.SemaphoreType.DMA((N_DEV - 1, nc)),
        ],
        compiler_params=_compiler_params(),
    )(x, gamma.reshape(1, n))
```
